```python
import numpy as np

kernel_name = "dist_ar_i_i_m2048_n512"

def setup_inputs():
    return {"x": np.random.randn(8192, 512).astype(np.float32)}

def reference(x: np.ndarray) -> np.ndarray:
    return x.reshape(4, 2048, 512).sum(axis=0)
```

```python
import jax
import jax.numpy as jnp
from jax import lax
from jax.experimental import pallas as pl
from jax.experimental.pallas import tpu as pltpu

MESH = pl.DeviceIdType.MESH
M, N = 2048, 512
Q = M // 4


def _spans(sizes):
    out, s = [], 0
    for n in sizes:
        out.append((s, n)); s += n
    assert s == Q, sizes
    return out


def make(c1=(32, 96, 128, 256), c2=(256, 256), c3=(256, 128, 64, 32, 32), step=64):
    s1, s2, s3 = _spans(c1), _spans(c2), _spans(c3)

    def body(x_hbm, o_hbm, xs, xk, t1, r1, t2, r2, t3, r3, ok, og,
             lsem, ksem, s1s, s1r, s2s, s2r, s3s, s3r, osem, gsem):
        me = lax.axis_index("i")
        cy = (me ^ (me >> 1)) & 1
        cx = me >> 1
        py, px = me ^ 1, 3 - me
        bar = pltpu.get_barrier_semaphore()
        for n in (py, px):
            pl.semaphore_signal(bar, inc=1, device_id=(n,), device_id_type=MESH)
        keep = (cy * Q, 2 * Q + cx * Q)
        give = ((1 - cy) * Q, 2 * Q + (1 - cx) * Q)
        pa = (py, px)
        pb = (px, py)

        def rows(base, s, n):
            return pl.ds(pl.multiple_of(base + s, 8), n)

        loads = [[pltpu.make_async_copy(x_hbm.at[rows(give[h], s, n)], xs.at[h, pl.ds(s, n)], lsem.at[h, i])
                  for h in range(2)] for i, (s, n) in enumerate(s1)]
        kloads = [pltpu.make_async_copy(x_hbm.at[rows(keep[h], 0, Q)], xk.at[h], ksem.at[h]) for h in range(2)]
        for row in loads:
            for c in row:
                c.start()
        for c in kloads:
            c.start()

        def rc(src, dst, ss, rs, spans, partner):
            return [[pltpu.make_async_remote_copy(src.at[h, pl.ds(s, n)], dst.at[h, pl.ds(s, n)], ss.at[h, i], rs.at[h, i],
                                                  device_id=(partner[h],), device_id_type=MESH)
                     for h in range(2)] for i, (s, n) in enumerate(spans)]

        p1 = rc(t1, r1, s1s, s1r, s1, pa)
        p2 = rc(t2, r2, s2s, s2r, s2, pb)
        p3 = rc(t3, r3, s3s, s3r, s3, pa)

        def tiles(s, n, f):
            for o in range(s, s + n, step):
                f(pl.ds(o, min(step, s + n - o)))

        for i, (s, n) in enumerate(s1):
            for h in range(2):
                loads[i][h].wait()
                def f(d, h=h):
                    t1[h, d] = xs[h, d].astype(jnp.bfloat16)
                tiles(s, n, f)
                if i > 0:
                    p1[i][h].start()
            if i == 0:
                pl.semaphore_wait(bar, 2)
                for h in range(2):
                    p1[0][h].start()
        for c in kloads:
            c.wait()

        def waiter(copies, spans):
            done = [0, 0]
            def upto(h, end):
                while done[h] < len(spans) and spans[done[h]][0] < end:
                    copies[done[h]][h].wait_recv()
                    done[h] += 1
            return upto

        w1, w2 = waiter(p1, s1), waiter(p2, s2)
        for i, (s, n) in enumerate(s2):
            for h in range(2):
                w1(h, s + n)
                def f(d, h=h):
                    t2[h, d] = (xk[h, d] + r1[h, d].astype(jnp.float32)).astype(jnp.bfloat16)
                tiles(s, n, f)
                p2[i][h].start()
        outs = []
        for i, (s, n) in enumerate(s3):
            for h in range(2):
                w2(h, s + n)
                def f(d, h=h):
                    v = (t2[h, d].astype(jnp.float32) + r2[h, d].astype(jnp.float32)).astype(jnp.bfloat16)
                    t3[h, d] = v
                    ok[h, d] = v.astype(jnp.float32)
                tiles(s, n, f)
                p3[i][h].start()
        for h in range(2):
            c = pltpu.make_async_copy(ok.at[h], o_hbm.at[rows(keep[h], 0, Q)], osem.at[h])
            c.start()
            outs.append(c)
        for i, (s, n) in enumerate(s3):
            for h in range(2):
                p3[i][h].wait_recv()
                def f(d, h=h):
                    og[h, d] = r3[h, d].astype(jnp.float32)
                tiles(s, n, f)
                c = pltpu.make_async_copy(og.at[h, pl.ds(s, n)], o_hbm.at[rows(give[h], s, n)], gsem.at[h, i])
                c.start()
                outs.append(c)
            if i == 0:
                for p in (p1, p2):
                    for row in p:
                        for c in row:
                            c.wait_send()
        for row in p3:
            for c in row:
                c.wait_send()
        for c in outs:
            c.wait()

    def fn(x):
        bf = lambda: pltpu.VMEM((2, Q, N), jnp.bfloat16)
        f32 = lambda: pltpu.VMEM((2, Q, N), jnp.float32)
        dma = pltpu.SemaphoreType.DMA
        return pl.pallas_call(
            body,
            out_shape=pltpu.HBM((M, N), jnp.float32),
            in_specs=[pl.BlockSpec(memory_space=pltpu.HBM)],
            out_specs=pl.BlockSpec(memory_space=pltpu.HBM),
            scratch_shapes=[f32(), f32(), bf(), bf(), bf(), bf(), bf(), bf(), f32(), f32(),
                            dma((2, len(s1))), dma((2,)),
                            dma((2, len(s1))), dma((2, len(s1))), dma((2, len(s2))), dma((2, len(s2))),
                            dma((2, len(s3))), dma((2, len(s3))), dma((2,)), dma((2, len(s3)))],
            compiler_params=pltpu.CompilerParams(collective_id=0, vmem_limit_bytes=48 * 1024 * 1024),
        )(x)
    return fn


pallas_dist_ar_i_i_m2048_n512_kernel = make()
```

```python
import jax
import jax.numpy as jnp
from jax import lax
from jax.experimental import pallas as pl
from jax.experimental.pallas import tpu as pltpu

MESH = pl.DeviceIdType.MESH
M, N = 2048, 512
Q = M // 4


def _spans(sizes):
    out, s = [], 0
    for n in sizes:
        out.append((s, n)); s += n
    assert s == Q, sizes
    return out


def make(c1=(32, 224, 256), c2=(256, 256), c3=(256, 256), step=64):
    s1, s2, s3 = _spans(c1), _spans(c2), _spans(c3)

    def body(x_hbm, o_ref, xs, xk, t1, r1, t2, r2, lsem, ksem, s1s, s1r, s2s, s2r, s3s, s3r):
        me = lax.axis_index("i")
        cy = (me ^ (me >> 1)) & 1
        cx = me >> 1
        py, px = me ^ 1, 3 - me
        bar = pltpu.get_barrier_semaphore()
        for n in (py, px):
            pl.semaphore_signal(bar, inc=1, device_id=(n,), device_id_type=MESH)
        keep = (cy * Q, 2 * Q + cx * Q)
        give = ((1 - cy) * Q, 2 * Q + (1 - cx) * Q)
        pa = (py, px)
        pb = (px, py)

        def rows(base, s, n):
            return pl.ds(pl.multiple_of(base + s, 16), n)

        loads = [[pltpu.make_async_copy(x_hbm.at[rows(give[h], s, n)], xs.at[h, pl.ds(s, n)], lsem.at[h, i])
                  for h in range(2)] for i, (s, n) in enumerate(s1)]
        kloads = [pltpu.make_async_copy(x_hbm.at[rows(keep[h], 0, Q)], xk.at[h], ksem.at[h]) for h in range(2)]
        for row in loads:
            for c in row:
                c.start()
        for c in kloads:
            c.start()

        def rc(src, dst, ss, rs, spans, partner):
            return [[pltpu.make_async_remote_copy(src.at[h, pl.ds(s, n)], dst.at[h, pl.ds(s, n)], ss.at[h, i], rs.at[h, i],
                                                  device_id=(partner[h],), device_id_type=MESH)
                     for h in range(2)] for i, (s, n) in enumerate(spans)]

        p1 = rc(t1, r1, s1s, s1r, s1, pa)
        p2 = rc(t2, r2, s2s, s2r, s2, pb)
        p3 = [[pltpu.make_async_remote_copy(o_ref.at[rows(keep[h], s, n)], o_ref.at[rows(keep[h], s, n)], s3s.at[h, i], s3r.at[h, i],
                                            device_id=(pa[h],), device_id_type=MESH)
               for h in range(2)] for i, (s, n) in enumerate(s3)]

        def tiles(s, n, f):
            for o in range(s, s + n, step):
                f(o, min(step, s + n - o))

        for i, (s, n) in enumerate(s1):
            for h in range(2):
                loads[i][h].wait()
                def f(o, k, h=h):
                    t1[h, pl.ds(o, k)] = xs[h, pl.ds(o, k)].astype(jnp.bfloat16)
                tiles(s, n, f)
                if i > 0:
                    p1[i][h].start()
            if i == 0:
                pl.semaphore_wait(bar, 2)
                for h in range(2):
                    p1[0][h].start()
        for c in kloads:
            c.wait()

        def waiter(copies, spans):
            done = [0, 0]
            def upto(h, end):
                while done[h] < len(spans) and spans[done[h]][0] < end:
                    copies[done[h]][h].wait_recv()
                    done[h] += 1
            return upto

        w1, w2 = waiter(p1, s1), waiter(p2, s2)
        for i, (s, n) in enumerate(s2):
            for h in range(2):
                w1(h, s + n)
                def f(o, k, h=h):
                    d = pl.ds(o, k)
                    t2[h, d] = (xk[h, d] + r1[h, d].astype(jnp.float32)).astype(jnp.bfloat16)
                tiles(s, n, f)
                p2[i][h].start()
        for i, (s, n) in enumerate(s3):
            for h in range(2):
                w2(h, s + n)
                def f(o, k, h=h):
                    d = pl.ds(o, k)
                    o_ref[rows(keep[h], o, k)] = (t2[h, d].astype(jnp.float32) + r2[h, d].astype(jnp.float32)).astype(jnp.bfloat16)
                tiles(s, n, f)
                p3[i][h].start()
        for p in (p1, p2, p3):
            for row in p:
                for c in row:
                    c.wait_send()
        for i, (s, n) in enumerate(s3):
            for h in range(2):
                d = o_ref.at[rows(give[h], s, n)]
                pltpu.make_async_remote_copy(d, d, s3s.at[h, i], s3r.at[h, i], device_id=(pa[h],), device_id_type=MESH).wait_recv()

    def fn(x):
        bf = lambda: pltpu.VMEM((2, Q, N), jnp.bfloat16)
        f32 = lambda: pltpu.VMEM((2, Q, N), jnp.float32)
        dma = pltpu.SemaphoreType.DMA
        return pl.pallas_call(
            body,
            out_shape=jax.ShapeDtypeStruct((M, N), jnp.bfloat16),
            in_specs=[pl.BlockSpec(memory_space=pltpu.HBM)],
            out_specs=pl.BlockSpec(memory_space=pltpu.VMEM),
            scratch_shapes=[f32(), f32(), bf(), bf(), bf(), bf(),
                            dma((2, len(s1))), dma((2,)),
                            dma((2, len(s1))), dma((2, len(s1))), dma((2, len(s2))), dma((2, len(s2))),
                            dma((2, len(s3))), dma((2, len(s3)))],
            compiler_params=pltpu.CompilerParams(collective_id=0),
        )(x)
    return fn


pallas_dist_ar_i_i_m2048_n512_kernel = make()
```

```python
import jax
import jax.numpy as jnp
import numpy as np
from jax import lax
from jax.experimental import pallas as pl
from jax.experimental.pallas import tpu as pltpu

MESH = pl.DeviceIdType.MESH
M, N = 2048, 512
E = M // 8
TILE = 32
I32 = jnp.int32


def _c(v):
    return np.array(v & 0xFFFFFFFF, np.uint32).view(np.int32)[()]


srl = lax.shift_right_logical
sll = lax.shift_left


def _shr(a, k):
    return srl(a, jnp.full(a.shape, k, I32))


def _shl(a, k):
    return sll(a, jnp.full(a.shape, k, I32))


def _encode_tile(w, bias):
    u = [x + bias for x in w]
    carry = u[0] ^ w[0]
    for x, y in zip(u[1:], w[1:]):
        carry = carry | (x ^ y)
    hi = lo = acc = None
    for j, x in enumerate(u):
        t = _shr(x, 9) & _c(0x003F003F)
        acc = t if acc is None else acc + t
        p = _c(63 * (j + 1) * 0x10001) - acc
        one = jnp.full(x.shape, _c(0x80000000 >> j), I32)
        a, b = srl(one, _shr(p, 16)), srl(one, p & _c(0xFFFF))
        hi = a if hi is None else hi | a
        lo = b if lo is None else lo | b
    n_hi = _shr(p, 16) + 8
    unary = hi | srl(lo, n_hi)
    length = n_hi + (p & _c(0xFFFF)) + 8
    a, b, c = u[5:]
    keep, six = _c(0x81FF81FF), _c(0x7E007E00)
    fixed = [
        (u[0] & keep) | (_shl(a, 9) & six),
        (u[1] & keep) | (_shl(b, 9) & six),
        (u[2] & keep) | (_shl(c, 9) & six),
        (u[3] & keep) | (_shl(a, 3) & _c(0x0E000E00)) | (_shl(b, 6) & _c(0x70007000)),
        (u[4] & keep) | (_shl(c, 3) & _c(0x0E000E00)) | (_shr(a, 1) & _c(0x40004000))
        | (_shr(b, 2) & _c(0x20002000)) | (_shr(c, 3) & _c(0x10001000)),
    ]
    return fixed, unary, length, carry


def _decode_tile(f, s, unbias):
    keep, six, three, sign = _c(0x81FF81FF), _c(0x003F003F), _c(0x01C001C0), _c(0x80008000)
    raw = [x & keep for x in f] + [
        (_shr(f[0], 9) & six) | (_shr(f[3], 3) & three) | (_shl(f[4], 1) & sign),
        (_shr(f[1], 9) & six) | (_shr(f[3], 6) & three) | (_shl(f[4], 2) & sign),
        (_shr(f[2], 9) & six) | (_shr(f[4], 3) & three) | (_shl(f[4], 3) & sign),
    ]
    q = []
    for _ in range(16):
        z = lax.clz(s)
        s = sll(_shl(s, 1), z)
        q.append(z)
    qq = [_shl(q[j], 25) | _shl(q[8 + j], 9) for j in range(8)]
    tot = qq[0]
    for x in qq[1:]:
        tot = tot + x
    used = _shr(tot, 25) + (_shr(tot, 9) & _c(0xFFFF)) + 16
    return [r + unbias - x for r, x in zip(raw, qq)], s, used


class _Msg:
    def __init__(self, row, rows, off, group):
        self.row, self.rows, self.off = row, rows, off
        self.tiles = rows // TILE
        self.groups = []
        t = 0
        while t < self.tiles:
            g = group if self.tiles - t >= group > 1 else 1
            self.groups.append((t, g))
            t += g
        self.short = sum(5 * g + max(g - 1, 1) for _, g in self.groups)
        self.size = 8 * (8 * self.tiles + 1)


def _stream(sizes, group):
    out, row, off = [], 0, 0
    for n in sizes:
        assert n % TILE == 0
        m = _Msg(row, n, off, group)
        out.append(m)
        row += n
        off += m.size
    assert row == E
    return out, off


DEFAULT_ORDER = ("a0 bar A0 a1 A1 a2 A2 b0 B0 b1 c0 C0 B1 c1 C1 t0 D0 E0 t1 D1 E1 t2 D2 E2 "
                 "F0 d0 e0 F1 d1 e1 F2 d2 e2 w f0 f1 f2")


def make(ca=(32, 96, 128), cb=(128, 128), cc=(128, 128), ct=(128, 96, 32), order=DEFAULT_ORDER, group=4,
         force_raw=False, **cp):
    streams = {"a": _stream(ca, group), "b": _stream(cb, group), "c": _stream(cc, group), "t": _stream(ct, group)}
    kind = {"A": "a", "B": "b", "C": "c", "D": "t", "E": "t", "F": "t"}
    tx_names, rx_names = "abct", "ABCDEF"
    sem_base, nsem = {}, 0
    for k in rx_names:
        sem_base[k] = nsem
        nsem += len(streams[kind[k]][0])
    nload = len(ca) + len(cb) + 2

    def body(x_hbm, o_ref, xv, words, dec, t_a, t_b, t_c, t_t, r_a, r_b, r_c, r_d, r_e, r_f, mode, lsem, ss, rs, ss2, rs2):
        tx = dict(zip(tx_names, (t_a, t_b, t_c, t_t)))
        rx = dict(zip(rx_names, (r_a, r_b, r_c, r_d, r_e, r_f)))
        me = lax.axis_index("i")
        cy, cx = (me ^ (me >> 1)) & 1, me >> 1
        py, px = me ^ 1, 3 - me
        bar = pltpu.get_barrier_semaphore()
        for n in (py, px):
            pl.semaphore_signal(bar, inc=1, device_id=(n,), device_id_type=MESH)
        first, second = (cy, cx), (cx, cy)
        peer = {k: (py, px) if k in "ABEF" else (px, py) for k in rx_names}

        def base(k, h):
            a, b = first[h], second[h]
            a = 1 - a if k in "abEF" else a
            b = 1 - b if k in "acDF" else b
            return (4 * h + 2 * a + b) * E

        def rows(k, h, s, n):
            return pl.ds(pl.multiple_of(base(k, h) + s, TILE), n)

        loads, j = {}, 0
        for k in "abct":
            parts = [(m.row, m.rows) for m in streams[k][0]] if k in "ab" else [(0, E)]
            for i, (s, n) in enumerate(parts):
                for h in range(2):
                    c = pltpu.make_async_copy(x_hbm.at[rows(k, h, s, n)], xv.at[h, tx_names.index(k), pl.ds(s, n)], lsem.at[h, j])
                    c.start()
                    loads[k, i, h] = c
                j += 1

        def copies(k, i, h):
            m = streams[kind[k]][0][i]
            src = rx["D"] if k == "F" else tx[kind[k]]
            j = sem_base[k] + i
            head = pl.ds(m.off + 7, 8 * m.short + 1)
            tail = pl.ds(m.off + 8 + 8 * m.short, 8 * (8 * m.tiles - m.short))
            return [pltpu.make_async_remote_copy(src.at[h, d], rx[k].at[h, d], s.at[h, j], r.at[h, j],
                                                 device_id=(peer[k][h],), device_id_type=MESH)
                    for d, s, r in ((head, ss, rs), (tail, ss2, rs2))]

        def slot(m, v):
            return pl.ds(m.off + 8 + 8 * v, 8)

        arrived, decoded, started = {}, set(), []

        def arrive(k, i, h):
            if (k, i, h) not in arrived:
                m = streams[kind[k]][0][i]
                head, tail = copies(k, i, h)
                head.wait_recv()
                hdr = rx[k][h, pl.ds(m.off + 7, 1)]
                plain = hdr[0, 0] < 0
                pl.when(plain)(tail.wait_recv)
                arrived[k, i, h] = (hdr, plain)
            return arrived[k, i, h]

        def unpack(k, i, h):
            if (k, i, h) in decoded:
                return
            decoded.add((k, i, h))
            m = streams[kind[k]][0][i]
            hdr, plain = arrive(k, i, h)
            src = rx[k]

            def put(t, w):
                for v, x in enumerate(w):
                    r, cols = m.row + t * TILE + 16 * (v // 4), pl.ds(128 * (v % 4), 128)
                    if k in "DEF":
                        o_ref[rows(k, h, r, 16), cols] = pltpu.bitcast(x, jnp.bfloat16)
                    else:
                        dec[h, "ABC".index(k), pl.ds(r // 2, 8), cols] = x

            @pl.when(plain)
            def _():
                for t in range(m.tiles):
                    put(t, [src[h, slot(m, 8 * t + v)] for v in range(8)])

            @pl.when(jnp.logical_not(plain))
            def _():
                unbias = jnp.broadcast_to(_c(0x7E007E00) - hdr, (8, 128))
                v = 0
                for t0, g in m.groups:
                    fixed = [[src[h, slot(m, v + 5 * t + e)] for e in range(5)] for t in range(g)]
                    v += 5 * g
                    rest = free = None
                    for t in range(max(g - 1, 1)):
                        w, left, used = _decode_tile(fixed[t], src[h, slot(m, v)], unbias)
                        v += 1
                        put(t0 + t, w)
                        rest = left if t == 0 else rest | jnp.where(free < 32, srl(left, free), 0)
                        free = 32 - used if t == 0 else free + (32 - used)
                    if g > 1:
                        put(t0 + g - 1, _decode_tile(fixed[g - 1], rest, unbias)[0])

        def pack(k, i, h):
            m = streams[k][0][i]
            ki = tx_names.index(k)
            c = loads.pop((k, i if k in "ab" else 0, h), None)
            if c is not None:
                c.wait()
            terms = {"a": "", "b": "", "c": "A", "t": "BC"}[k]
            for r in terms:
                for i2, m2 in enumerate(streams[kind[r]][0]):
                    if m2.row < m.row + m.rows and m.row < m2.row + m2.rows:
                        unpack(r, i2, h)
            top = None
            for r in range(m.row, m.row + m.rows, 16):
                v = xv[h, ki, pl.ds(r, 16)]
                for s in terms:
                    v = v + pltpu.bitcast(dec[h, "ABC".index(s), pl.ds(r // 2, 8)], jnp.bfloat16).astype(jnp.float32)
                b = v.astype(jnp.bfloat16)
                words[pl.ds((r - m.row) // 2, 8)] = pltpu.bitcast(b, I32)
                if k == "t":
                    o_ref[rows(k, h, r, 16)] = b
                a = jnp.abs(v)
                a = jnp.maximum(a[:, :256], a[:, 256:])
                a = jnp.maximum(a[:, :128], a[:, 128:])
                top = a if top is None else jnp.maximum(top, a)
            top = jnp.max(top, axis=0, keepdims=True)
            top = _shr(pltpu.bitcast(jnp.broadcast_to(top, (8, 128)), I32) + 0xFFFF, 16) & 0x7FFF
            bias = 0x7FFF - top
            bias = bias | _shl(bias, 16)
            dst = tx[k]

            def tile(t):
                return [words[pl.ds(16 * t + 8 * (v // 4), 8), pl.ds(128 * (v % 4), 128)] for v in range(8)]

            v, carry, spare = 0, None, None
            for t0, g in m.groups:
                enc = [_encode_tile(tile(t0 + t), bias) for t in range(g)]
                for f, _, n, cr in enc:
                    for x in f:
                        dst[h, slot(m, v)] = x
                        v += 1
                    carry = cr if carry is None else carry | cr
                    spare = 31 - n if spare is None else spare | (31 - n)
                rest, left = (enc[-1][1], enc[-1][2]) if g > 1 else (None, None)
                for _, s, n, _ in enc[:max(g - 1, 1)]:
                    if g > 1:
                        s = s | srl(rest, n)
                        rest, left = sll(rest, 32 - n), left - (32 - n)
                    dst[h, slot(m, v)] = s
                    v += 1
                if g > 1:
                    spare = spare | -left
            bad = ((carry & _c(0x80008000)) != 0) | (spare < 0)
            plain = jnp.max(jnp.where(bad, 1.0, 0.0)) > (-1.0 if force_raw else 0.0)
            dst[h, pl.ds(m.off, 8)] = jnp.where(plain, -1, bias)
            mode[ki, h, i] = plain.astype(I32)

            @pl.when(plain)
            def _():
                for t in range(m.tiles):
                    for e, x in enumerate(tile(t)):
                        dst[h, slot(m, 8 * t + e)] = x

        def send(k, i, h):
            plain = arrive("D", i, h)[1] if k == "F" else mode[tx_names.index(kind[k]), h, i] != 0
            head, tail = copies(k, i, h)
            head.start()
            pl.when(plain)(tail.start)
            started.append((head, tail, plain))

        def drain():
            for head, tail, plain in started:
                head.wait_send()
                pl.when(plain)(tail.wait_send)
            started.clear()

        for op in order.split():
            if op == "bar":
                pl.semaphore_wait(bar, 2)
            elif op == "w":
                drain()
            else:
                k, i = op[0], int(op[1])
                for h in ((0, 1) if len(op) == 2 else (int(op[2]),)):
                    if k in tx_names:
                        pack(k, i, h)
                    elif k in "def":
                        unpack(k.upper(), i, h)
                    elif k in "pqr":
                        unpack("ABC"["pqr".index(k)], i, h)
                    else:
                        send(k, i, h)
        drain()

    def fn(x):
        dma = pltpu.SemaphoreType.DMA
        buf = lambda k: pltpu.VMEM((2, streams[k][1], 128), I32)
        return pl.pallas_call(
            body,
            out_shape=jax.ShapeDtypeStruct((M, N), jnp.bfloat16),
            in_specs=[pl.BlockSpec(memory_space=pltpu.HBM)],
            out_specs=pl.BlockSpec(memory_space=pltpu.VMEM),
            scratch_shapes=[pltpu.VMEM((2, 4, E, N), jnp.float32), pltpu.VMEM((E // 2, N), I32), pltpu.VMEM((2, 3, E // 2, N), I32),
                            *[buf(k) for k in tx_names], *[buf(kind[k]) for k in rx_names],
                            pltpu.SMEM((4, 2, 8), I32), dma((2, nload)),
                            dma((2, nsem)), dma((2, nsem)), dma((2, nsem)), dma((2, nsem))],
            compiler_params=pltpu.CompilerParams(collective_id=0, **{"disable_semaphore_checks": True, **cp}),
        )(x)
    return fn


pallas_dist_ar_i_i_m2048_n512_kernel = make()
```

```python
import functools
import operator

import jax
import jax.numpy as jnp
import numpy as np
from jax import lax
from jax.experimental import pallas as pl
from jax.experimental.pallas import tpu as pltpu

M, N = 2048, 512
BLOCK = M // 8
TILE = 32
I32 = jnp.int32
MESH = pl.DeviceIdType.MESH

CHUNKS = {"a": (1, 3, 3, 1), "b": (4, 3, 1), "c": (4, 3, 1), "t": (4, 4)}
STREAM = {"A": "a", "B": "b", "C": "c", "D": "t", "E": "t", "F": "t", "X": "a"}
TERMS = {"a": "", "b": "X", "c": "A", "t": "BC"}
APART = {("A", 0): 1, ("A", 1): 3, ("F", 1): 2}
MOVED = 3

SCHEDULE = """
    L4 bar:m bar:l go:l g00 G00:ml g01 G01:l L2 a0 A00:ml A01:l g10 G10:ml g11 G11:l
    rdy:m G01:m A01:m G11:m a1 bar:f G0:f A0:f G1:f A1 L a2 A2 a3 A3 b0 B0
    c0 C0 b1 B1 b2 B2 c1 C1 c2 C2 t0 D0 E0 t1 D1 E1 F0 d0 e0 F1 d1 e1 f0 w f1
"""

HEADER_BITS = 13
ROOM = {1: (1, 4), 3: (5, 3), 4: (6, 5)}
MAIN, MORE_POOL, LOW, MORE_HIGH = range(4)


def _i32(v):
    return np.array(v & 0xFFFFFFFF, np.uint32).view(np.int32)[()]


SIGNS, BYTES = _i32(0x80008000), _i32(0x00FF00FF)
_srl, _sll = lax.shift_right_logical, lax.shift_left


def _shr(x, k):
    return _srl(x, _i32(k)) if k else x


def _shl(x, k):
    return _sll(x, _i32(k)) if k else x


def _or(xs):
    return functools.reduce(operator.or_, xs)


def _row(like):
    return lax.broadcasted_iota(I32, like.shape, 1)


def _twice(offset):
    return jnp.concatenate([_shl(offset, 20) | _shl(offset, 4)] * 4, axis=2)


def _swap(x):
    return x ^ (_shr((x & _i32(0x7E807E80)) + _i32(0x01800180), 7) & _i32(0x01000100))


def _skew(x, sign):
    group, out = _row(x) & 3, x
    for g in range(1, 4):
        out = jnp.where(group == g, pltpu.roll(x, 32 * g * sign % 128, 2), out)
    return out


def _sum_above(x):
    row, total = _row(x), x
    for k in (1, 2, 4):
        total = total + jnp.where(row >= k, pltpu.roll(total, k, 1), 0)
    return total - x


def _words_at(run, last):
    return range(run // 4, min(run, (16 * run + 30) // 32, last) + 1)


class _Message:
    def __init__(self, row, tiles, start):
        self.row, self.tiles, self.rows, self.start = row, tiles, tiles * TILE, start
        units, self.pool_rows = ROOM[tiles]
        self.full, self.half = divmod(units, 2)
        self.signs = 4 * tiles
        self.unary = self.signs + (tiles + 1) // 2
        self.pool = self.unary + self.full
        self.size = 8 * tiles + 1

    def low(self, t, j):
        return 4 * (self.tiles - 1 - t) + j

    def high(self, t, j):
        v = self.signs + 4 * t + j
        return v + (v >= self.pool)

    def at(self, v, row=0, rows=8):
        return pl.ds(8 * (self.start + v) + row, rows)


def _messages(chunks):
    out, row, start = [], 0, 0
    for tiles in chunks:
        out.append(_Message(row, tiles, start))
        row, start = row + out[-1].rows, start + out[-1].size
    assert row == BLOCK
    return out


def _encode_high(m, tile, store, header):
    code = [[] for _ in range(m.full + m.half + 2)]
    spare, signs = [], []
    for t in range(m.tiles):
        words = tile(t)
        signs = [_or(signs + [_shr(w & SIGNS, 8 * (t % 2) + j) for j, w in enumerate(words)])]
        if t % 2:
            store(m.signs + t // 2, signs.pop())
        upper, lower = [], []
        for j, w in enumerate(words):
            field = _shr(w, 8) & _i32(0x007F007F)
            fields = field if j == 0 else fields + field
            zeros = _i32(127 * (j + 1) * 0x10001) - fields
            upper.append(_srl(_i32(0x80000000 >> j), _shr(zeros, 16)))
            lower.append(_srl(_i32(0x80000000 >> j), zeros & 0xFFFF))
        for run, bits, length in ((2 * t, _or(upper), _shr(zeros, 16) + 8),
                                  (2 * t + 1, _or(lower), (zeros & 0xFFFF) + 8)):
            spare.append(32 - length)
            if run == 0:
                code[0].append(bits)
                end = length
                continue
            allowed = _words_at(run, len(code) - 1)
            word, bit = _shr(end, 5), end & 31
            left, right = _srl(bits, bit), _sll(_shl(bits, 1), 31 - bit)
            for k in allowed:
                here = word == k
                code[k].append(jnp.where(here, left, 0))
                if k + 1 < len(code):
                    code[k + 1].append(jnp.where(here, right, 0))
            spare.append(allowed[-1] - word)
            end = end + length
        code = [[_or(x)] if x else [] for x in code]
        spare = [_or(spare)]
    code = [x[0] if x else jnp.zeros_like(end) for x in code]
    for k in range(m.full):
        store(m.unary + k, code[k])
    rest = code[m.full:]
    if m.half:
        store(m.unary - 1, signs.pop() | (_shr(rest[0], 8) & 0xFF0000) | (_shr(rest[0], 16) & 0xFF))
        rest = [_shl(a, 16) | _shr(b, 16) for a, b in zip(rest, rest[1:])]

    length = end - (32 * m.full + 16 * m.half)
    length = _skew(jnp.where(length > 0, length, 0), 1)
    first, second = (_skew(x, 1) for x in rest)
    start = _sum_above(length) + HEADER_BITS
    word, bit, row = _shr(start, 5), start & 31, _row(start)
    pieces = (_srl(first, bit), _sll(_shl(first, 1), 31 - bit) | _srl(second, bit),
              _sll(_shl(second, 1), 31 - bit))
    pool = jnp.where(row == 0, header, 0)
    for down in range(8):
        which, x = ((row + down) & 7) - word, 0
        for k, piece in enumerate(pieces):
            x = jnp.where(which == k, piece, x)
        pool = pool | (pltpu.roll(x, down, 1) if down else x)
    end = start + length
    fits = (spare[0] | (64 - length) | (256 - end)) >= 0
    return pool, jnp.where(fits, jnp.where(end > 32 * m.pool_rows, 1.0, 0.0), 2.0)


def _decode_high(m, load, pool):
    code = [load(m.unary + k) for k in range(m.full)]
    if m.half:
        x = load(m.unary - 1)
        code.append(_shl(x & 0xFF0000, 8) | _shl(x & 0xFF, 16))
    ones = functools.reduce(operator.add, [lax.population_count(x) for x in code])
    skip = _sum_above(_skew(16 * m.tiles - ones, 1)) + 1
    pool = [(pool[0] & _i32(0xFFFFFFFF >> HEADER_BITS)) | (1 << (32 - HEADER_BITS))] + pool[1:]
    near, left = pool[:3], skip
    for r in range(1, 8):
        left = left - lax.population_count(pool[r - 1])
        past = left > 0
        skip = jnp.where(past, left, skip)
        near = [jnp.where(past, a, b) for a, b in zip(pool[r:r + 3], near)] + near[8 - r:]
    x, bit = near[0], jnp.zeros_like(skip)
    for k in (16, 8, 4, 2, 1):
        left = skip - lax.population_count(_shr(x, 32 - k))
        past = left > 0
        skip, x = jnp.where(past, left, skip), jnp.where(past, _shl(x, k), x)
        bit = jnp.where(past, bit + k, bit)
    rest = [_skew(_sll(_shl(a, 1), bit) | _srl(b, 31 - bit), -1) for a, b in zip(near, near[1:])]
    if m.half:
        code[-1] = code[-1] | _shr(rest[0], 16)
        rest = [_shl(rest[0], 16) | _shr(rest[1], 16), _shl(rest[1], 16)]
    code += rest

    for t in range(m.tiles):
        zeros = []
        for run in (2 * t, 2 * t + 1):
            if run == 0:
                bits, end = code[0], 8
            else:
                allowed = _words_at(run, len(code) - 1)
                word, bit = _shr(end, 5), end & 31
                left, right = code[allowed[0]], code[allowed[0] + 1]
                for k in allowed[1:]:
                    here = word == k
                    left = jnp.where(here, code[k], left)
                    if k + 1 < len(code):
                        right = jnp.where(here, code[k + 1], right)
                bits, end = _sll(left, bit) | _srl(_shr(right, 1), 31 - bit), end + 8
            for _ in range(8):
                zeros.append(lax.clz(bits))
                bits, end = _sll(_shl(bits, 1), zeros[-1]), end + zeros[-1]
        signs = load(m.signs + t // 2)
        yield [(_shl(signs, 8 * (t % 2) + j) & SIGNS)
               | ((_shl(zeros[j], 24) | _shl(zeros[8 + j], 8)) ^ _i32(0x7F007F00)) for j in range(8)]


MESSAGES = {k: _messages(chunks) for k, chunks in CHUNKS.items()}
ENCODED = [(k, i) for k in CHUNKS for i in range(len(CHUNKS[k]))]
SENT = [(k, i) for k in "ABCDEF" for i in range(len(CHUNKS[STREAM[k]]))] + [("X", MOVED)]


def _steps():
    for step in SCHEDULE.split():
        step, _, chips = step.partition(":")
        name = step.rstrip("0123456789")
        digits = [int(d) for d in step[len(name):]]
        yield name, digits[0] if digits else None, digits[1:] or [0, 1], chips


def _body(x_hbm, out, own, terms, words, levels, ready, load_sems, send_sems, recv_sems, *buffers):
    outbox, inbox = dict(zip(CHUNKS, buffers)), dict(zip(STREAM, buffers[len(CHUNKS):]))
    me = lax.axis_index("i")
    neighbours = me ^ 1, 3 - me
    role = {"f": me == 0, "m": (me & 1) == 1, "l": me == 2}
    barrier = pltpu.get_barrier_semaphore()

    def signal(sem):
        for chip in neighbours:
            pl.semaphore_signal(sem, inc=1, device_id=(chip,), device_id_type=MESH)

    pl.when(me != 2)(lambda: signal(barrier))

    flip = (me == 3).astype(I32)
    half = flip, 1 - flip
    link = [jnp.where(h == 0, *neighbours) for h in half]
    place = [jnp.where(h == 0, (me ^ (me >> 1)) & 1, me >> 1) for h in half]

    def rows(k, u, row, n):
        a = 1 - place[u] if k in "abEF" else place[u]
        b = 1 - place[1 - u] if k in "acDF" else place[1 - u]
        return pl.ds(pl.multiple_of((4 * half[u] + 2 * a + b) * BLOCK + row, 16), n)

    loads = {}
    for k, i, halves, _ in _steps():
        k = "a" if k == "g" else k
        for u in halves if k in CHUNKS else ():
            if (k, i, u) not in loads:
                m = MESSAGES[k][i]
                loads[k, i, u] = pltpu.make_async_copy(
                    x_hbm.at[rows(k, u, m.row, m.rows)],
                    own.at[list(CHUNKS).index(k), u, pl.ds(m.row, m.rows)],
                    load_sems.at[len(loads)])
    waiting = list(loads.values())

    def copy(k, i, u, part, sending=False):
        m = MESSAGES[STREAM[k]][i]
        peer = link[u if k in "ABEF" else 1 - u]
        there = half[u] ^ (peer == 3).astype(I32) if sending else u
        cut, sent = 32 * APART.get((k, i), 0), 8 * m.pool + m.pool_rows
        lo, hi = {MAIN: (cut, sent), MORE_POOL: (sent, 8 * m.pool + 8), LOW: (0, cut),
                  MORE_HIGH: (8 * m.pool + 8, 8 * m.size)}[part]
        span, sem = m.at(0, lo, hi - lo), 4 * SENT.index((k, i)) + part
        source = inbox["D"] if k == "F" else outbox[STREAM[k]]
        return pltpu.make_async_remote_copy(
            source.at[u, span], inbox[k].at[there, span], send_sems.at[u, sem],
            recv_sems.at[there, sem], device_id=(peer,), device_id_type=MESH)

    def on_demand(level, f):
        @pl.when(level > 0)
        def _():
            pl.when(level == 1)(lambda: f(MORE_POOL))
            pl.when(level > 1)(lambda: f(MORE_HIGH))

    arrived, unfinished = {}, []

    def arrive(k, i, u):
        if (k, i, u) not in arrived:
            m = MESSAGES[STREAM[k]][i]
            copy(k, i, u, MAIN).wait_recv()
            level = _shr(inbox[k][u, m.at(m.pool, 0, 1)][0, 0], 30)
            on_demand(level, lambda part: copy(k, i, u, part).wait_recv())
            arrived[k, i, u] = level
        return arrived[k, i, u]

    def pairs(m, t, lower):
        return pl.ds((m.row + TILE * t) // 2 + 8 * lower, 8)

    def receive(k, i):
        m, box = MESSAGES[STREAM[k]][i], inbox[k]
        verbatim = [arrive(k, i, u) > 1 for u in range(2)]

        def pool_row(r):
            return jnp.broadcast_to(box[:, m.at(m.pool, r, 1)], (2, 8, 128))

        @pl.when(jnp.logical_not(jnp.logical_and(*verbatim)))
        def _():
            pool = [pool_row(r) for r in range(8)]
            more = _shr(pool[0], 30) == 1
            pool[m.pool_rows:] = [jnp.where(more, x, 0) for x in pool[m.pool_rows:]]
            for t, high in enumerate(_decode_high(m, lambda v: box[:, m.at(v)], pool)):
                for lower in range(2):
                    words[:, pairs(m, t, lower)] = jnp.concatenate(high[4 * lower:4 * lower + 4], axis=2)

        for u in range(2):
            @pl.when(verbatim[u])
            def _():
                for t in range(m.tiles):
                    high = jnp.concatenate([box[u, m.at(m.high(t, j))] for j in range(4)], axis=1)
                    words[u, pairs(m, t, 0)] = _shl(high & BYTES, 8)
                    words[u, pairs(m, t, 1)] = high & ~BYTES

        offset = _twice(_shr(pool_row(0), 32 - HEADER_BITS) & 0x7FF)
        for t in range(m.tiles):
            if t == m.tiles - APART.get((k, i), 0):
                for u in range(2):
                    copy(k, i, u, LOW).wait_recv()
            low = jnp.concatenate([box[:, m.at(m.low(t, j))] for j in range(4)], axis=2)
            for lower in range(2):
                x = _swap(words[:, pairs(m, t, lower)] | (_shr(low, 8 * lower) & BYTES)) - offset
                if k in "DEF":
                    for u in range(2):
                        row = m.row + TILE * t + 16 * lower
                        out[rows(k, u, row, 16)] = pltpu.bitcast(x[u], jnp.bfloat16)
                else:
                    terms["ABCX".index(k), :, pairs(m, t, lower)] = x

    def receive_term(k, i):
        if STREAM[k] != "a" or i != MOVED:
            return receive(k, i)
        comes = role["l"] if k == "X" else jnp.logical_not(role["f"])
        pl.when(comes)(lambda: receive(k, i))

        @pl.when(jnp.logical_not(comes))
        def _():
            m = MESSAGES["a"][i]
            terms["ABCX".index(k), :, pl.ds(m.row // 2, m.rows // 2)] = jnp.full(
                (2, m.rows // 2, N), SIGNS, I32)

    def encode_low(k, i, halves):
        m, span = MESSAGES[k][i], slice(halves[0], halves[-1] + 1)
        for u in halves:
            loads.pop((k, i, u)).wait()
        added = [(r, j) for r, j in SENT if r in TERMS[k]
                 and m.row <= MESSAGES[STREAM[r]][j].row < m.row + m.rows]
        for r, j in added:
            receive_term(r, j)
        tops = []
        for u in halves:
            for row in range(m.row, m.row + m.rows, 16):
                x = own[list(CHUNKS).index(k), u, pl.ds(row, 16)]
                for r in sorted({r for r, _ in added}):
                    term = terms["ABCX".index(r), u, pl.ds(row // 2, 8)]
                    x = x + pltpu.bitcast(term, jnp.bfloat16).astype(jnp.float32)
                rounded = x.astype(jnp.bfloat16)
                words[u, pl.ds(row // 2, 8)] = pltpu.bitcast(rounded, I32)
                if k == "t":
                    out[rows(k, u, row, 16)] = rounded
                x = jnp.abs(x)
                x = jnp.maximum(x[:, :256], x[:, 256:])
                x = jnp.maximum(x[:, :128], x[:, 128:])
                top = x if row == m.row else jnp.maximum(top, x)
            top = jnp.broadcast_to(jnp.max(top, axis=0, keepdims=True), (8, 128))
            tops.append(pltpu.bitcast(top, I32))
        offset = _shr(0x7FFF - (_shr(jnp.stack(tops) + 0xFFFF, 16) & 0x7FFF), 4)
        outbox[k][span, m.at(m.pool)] = _shl(offset, 32 - HEADER_BITS)
        offset = _twice(offset)
        for t in range(m.tiles):
            x = [_swap(words[span, pairs(m, t, lower)] + offset) for lower in range(2)]
            for lower in range(2):
                words[span, pairs(m, t, lower)] = x[lower]
            low = (x[0] & BYTES) | _shl(x[1] & BYTES, 8)
            for j in range(4):
                outbox[k][span, m.at(m.low(t, j))] = low[:, :, 128 * j:128 * (j + 1)]

    def encode(k, i):
        m, box = MESSAGES[k][i], outbox[k]
        if (k, i, 0) in loads:
            encode_low(k, i, [0, 1])

        def tile(t):
            return [words[:, pairs(m, t, j // 4), pl.ds(128 * (j % 4), 128)] for j in range(8)]

        def store(v, x):
            box[:, m.at(v)] = x

        pool, needs = _encode_high(m, tile, store, box[:, m.at(m.pool)])
        store(m.pool, pool)
        for u, level in enumerate([jnp.max(needs[u]).astype(I32) for u in range(2)]):
            levels[u, ENCODED.index((k, i))] = level

            @pl.when(level > 0)
            def _():
                first = m.at(m.pool, 0, 1)
                box[u, first] = (box[u, first] & 0x3FFFFFFF) | _shl(level, 30)

                @pl.when(level > 1)
                def _():
                    for t in range(m.tiles):
                        high = ((_shr(words[u, pairs(m, t, 0)], 8) & BYTES)
                                | (words[u, pairs(m, t, 1)] & ~BYTES))
                        for j in range(4):
                            box[u, m.at(m.high(t, j))] = high[:, 128 * j:128 * (j + 1)]

    def each_copy(k, i, u, f, low):
        level = arrive("D", i, u) if k == "F" else levels[u, ENCODED.index((STREAM[k], i))]

        def to(k):
            f(copy(k, i, u, MAIN, True))
            on_demand(level, lambda part: f(copy(k, i, u, part, True)))
            if low and (k, i) in APART:
                f(copy(k, i, u, LOW, True))

        if (k, i, u) == ("A", MOVED, 0):
            pl.when(role["m"])(lambda: to("X"))
            pl.when(jnp.logical_not(role["m"]))(lambda: to("A"))
        else:
            to(k)

    def finish_sends(keep):
        while len(unfinished) > keep:
            each_copy(*unfinished.pop(0), lambda c: c.wait_send(), True)

    def run(name, i, halves, chips):
        if name == "L":
            for c in waiting[:i]:
                c.start()
            del waiting[:i]
        elif name == "bar":
            pl.semaphore_wait(barrier, 1 if chips == "m" else 2)
        elif name == "go":
            signal(ready)
        elif name == "rdy":
            pl.semaphore_wait(ready, 1)
        elif name == "w":
            finish_sends(2)
        elif name == "g":
            encode_low("a", i, halves)
        elif name == "G":
            for u in halves:
                copy("A", i, u, LOW, True).start()
        elif name in CHUNKS:
            encode(name, i)
        elif name in STREAM:
            for u in halves:
                each_copy(name, i, u, lambda c: c.start(), name != "A")
                if (name, i, u) not in unfinished:
                    unfinished.append((name, i, u))
        else:
            receive(name.upper(), i)

    for step in _steps():
        if step[-1]:
            chosen = functools.reduce(jnp.logical_or, [role[r] for r in step[-1]])
            pl.when(chosen)(functools.partial(run, *step))
        else:
            run(*step)
    finish_sends(0)
    assert not waiting and not loads


def pallas_dist_ar_i_i_m2048_n512_kernel(x: jax.Array):
    assert x.shape == (M, N) and x.dtype == jnp.float32

    def box(k):
        return pltpu.VMEM((2, 8 * sum(m.size for m in MESSAGES[k]), 128), I32)

    return pl.pallas_call(
        _body,
        out_shape=jax.ShapeDtypeStruct((M, N), jnp.bfloat16),
        in_specs=[pl.BlockSpec(memory_space=pltpu.HBM)],
        out_specs=pl.BlockSpec(memory_space=pltpu.VMEM),
        scratch_shapes=[
            pltpu.VMEM((4, 2, BLOCK, N), jnp.float32),
            pltpu.VMEM((4, 2, BLOCK // 2, N), I32),
            pltpu.VMEM((2, BLOCK // 2, N), I32),
            pltpu.SMEM((2, len(ENCODED)), I32),
            pltpu.SemaphoreType.REGULAR,
            pltpu.SemaphoreType.DMA((2 * len(ENCODED),)),
            pltpu.SemaphoreType.DMA((2, 4 * len(SENT))),
            pltpu.SemaphoreType.DMA((2, 4 * len(SENT))),
            *[box(k) for k in CHUNKS],
            *[box(k) for k in STREAM.values()],
        ],
        compiler_params=pltpu.CompilerParams(collective_id=0, disable_semaphore_checks=True),
    )(x)
```

```python
import functools
import operator

import jax
import jax.numpy as jnp
import numpy as np
from jax import lax
from jax.experimental import pallas as pl
from jax.experimental.pallas import tpu as pltpu

M, N = 2048, 512
BLOCK = M // 8
TILE = 32
I32 = jnp.int32
MESH = pl.DeviceIdType.MESH

CHUNKS = {"a": (1, 3, 3, 1), "b": (4, 3, 1), "c": (4, 3, 1), "t": (4, 4)}
STREAM = {"A": "a", "B": "b", "C": "c", "D": "t", "E": "t", "F": "t", "X": "a"}
TERMS = {"a": "", "b": "X", "c": "A", "t": "BC"}
APART = {("A", 0): 1, ("A", 1): 3, ("C", 0): 4, ("E", 0): 4, ("E", 1): 4, ("F", 1): 2}
MOVED = 3

SCHEDULE = """
    load4 bar:m bar:l go:l a-00 A-00:ml a-01 A-01:l load2 a0 A00:ml A01:l
    a-10 A-10:ml a-11 A-11:l rdy:m A-01:m A01:m A-11:m a1 bar:f A-0:f A0:f A-1:f A1
    load4 a2 A2 load a3 A3 b0 B0 c-0 C-0 c0 C0 b1 B1 b2 B2 c1 C1 c2 C2
    t-0 E-0 t0 D0 E0 t-1 E-1 t1 D1 E1 F0 d0 e0 F1 d1 e1 f0 sent f1
"""

HEADER_BITS = 13
ROOM = {1: (1, 4), 3: (5, 2), 4: (6, 5)}
MAIN, POOL_ROW, POOL_REST, HIGH_BYTES, LOW = range(5)


def _i32(v):
    return np.array(v & 0xFFFFFFFF, np.uint32).view(np.int32)[()]


SIGNS, BYTES = _i32(0x80008000), _i32(0x00FF00FF)
_srl, _sll = lax.shift_right_logical, lax.shift_left


def _shr(x, k):
    return _srl(x, _i32(k)) if k else x


def _shl(x, k):
    return _sll(x, _i32(k)) if k else x


def _or(xs):
    return functools.reduce(operator.or_, xs)


def _row(like):
    return lax.broadcasted_iota(I32, like.shape, 1)


def _twice(offset):
    return jnp.concatenate([_shl(offset, 20) | _shl(offset, 4)] * 4, axis=2)


def _swap(x):
    return x ^ (_shr((x & _i32(0x7E807E80)) + _i32(0x01800180), 7) & _i32(0x01000100))


def _skew(m, x, sign):
    if m.tiles == 1:
        return x
    group, out = _row(x) & 3, x
    for g in range(1, 4):
        out = jnp.where(group == g, pltpu.roll(x, 32 * g * sign % 128, 2), out)
    return out


def _sum_above(x):
    row, total = _row(x), x
    for k in (1, 2, 4):
        total = total + jnp.where(row >= k, pltpu.roll(total, k, 1), 0)
    return total - x


def _words_at(run, last):
    return range(run // 4, min(run, (16 * run + 30) // 32, last) + 1)


class _Message:
    def __init__(self, row, tiles, start):
        self.row, self.tiles, self.rows, self.start = row, tiles, tiles * TILE, start
        units, self.pool_rows = ROOM[tiles]
        self.full, self.half = divmod(units, 2)
        self.signs = 4 * tiles
        self.unary = self.signs + (tiles + 1) // 2
        self.pool = self.unary + self.full
        self.size = 8 * tiles + 1

    def low(self, t, j):
        return 4 * (self.tiles - 1 - t) + j

    def high(self, t, j):
        v = self.signs + 4 * t + j
        return v + (v >= self.pool)

    def at(self, v, row=0, rows=8):
        return pl.ds(8 * (self.start + v) + row, rows)


def _messages(chunks):
    out, row, start = [], 0, 0
    for tiles in chunks:
        out.append(_Message(row, tiles, start))
        row, start = row + out[-1].rows, start + out[-1].size
    assert row == BLOCK
    return out


def _encode_high(m, tile, store, header):
    code = [[] for _ in range(m.full + m.half + 2)]
    spare, signs = [], []
    for t in range(m.tiles):
        words = tile(t)
        signs = [_or(signs + [_shr(w & SIGNS, 8 * (t % 2) + j) for j, w in enumerate(words)])]
        if t % 2:
            store(m.signs + t // 2, signs.pop())
        upper, lower = [], []
        for j, w in enumerate(words):
            field = _shr(w, 8) & _i32(0x007F007F)
            fields = field if j == 0 else fields + field
            zeros = _i32(127 * (j + 1) * 0x10001) - fields
            upper.append(_srl(_i32(0x80000000 >> j), _shr(zeros, 16)))
            lower.append(_srl(_i32(0x80000000 >> j), zeros & 0xFFFF))
        for run, bits, length in ((2 * t, _or(upper), _shr(zeros, 16) + 8),
                                  (2 * t + 1, _or(lower), (zeros & 0xFFFF) + 8)):
            spare.append(32 - length)
            if run == 0:
                code[0].append(bits)
                end = length
                continue
            allowed = _words_at(run, len(code) - 1)
            word, bit = _shr(end, 5), end & 31
            left, right = _srl(bits, bit), _sll(_shl(bits, 1), 31 - bit)
            for k in allowed:
                here = word == k
                code[k].append(jnp.where(here, left, 0))
                if k + 1 < len(code):
                    code[k + 1].append(jnp.where(here, right, 0))
            spare.append(allowed[-1] - word)
            end = end + length
        code = [[_or(x)] if x else [] for x in code]
        spare = [_or(spare)]
    code = [x[0] if x else jnp.zeros(end.shape, I32) for x in code]
    for k in range(m.full):
        store(m.unary + k, code[k])
    rest = code[m.full:]
    if m.half:
        store(m.unary - 1, signs.pop() | (_shr(rest[0], 8) & 0xFF0000) | (_shr(rest[0], 16) & 0xFF))
        rest = [_shl(a, 16) | _shr(b, 16) for a, b in zip(rest, rest[1:])]

    length = end - (32 * m.full + 16 * m.half)
    length = _skew(m, jnp.where(length > 0, length, 0), 1)
    first, second = (_skew(m, x, 1) for x in rest)
    start = _sum_above(length) + HEADER_BITS
    word, bit, row = _shr(start, 5), start & 31, _row(start)
    pieces = (_srl(first, bit), _sll(_shl(first, 1), 31 - bit) | _srl(second, bit),
              _sll(_shl(second, 1), 31 - bit))
    pool = jnp.where(row == 0, header, 0)
    for down in range(8):
        which, x = ((row + down) & 7) - word, 0
        for k, piece in enumerate(pieces):
            x = jnp.where(which == k, piece, x)
        pool = pool | (pltpu.roll(x, down, 1) if down else x)
    end = start + length
    fits = (spare[0] | (64 - length) | (256 - end)) >= 0
    level = jnp.where(end > 32 * m.pool_rows, float(POOL_ROW), float(MAIN))
    level = jnp.where(end > 32 * (m.pool_rows + 1), float(POOL_REST), level)
    return pool, jnp.where(fits, level, float(HIGH_BYTES))


def _decode_high(m, load, pool):
    code = [load(m.unary + k) for k in range(m.full)]
    if m.half:
        x = load(m.unary - 1)
        code.append(_shl(x & 0xFF0000, 8) | _shl(x & 0xFF, 16))
    ones = functools.reduce(operator.add, [lax.population_count(x) for x in code])
    skip = _sum_above(_skew(m, 16 * m.tiles - ones, 1)) + 1
    pool = [(pool[0] & _i32(0xFFFFFFFF >> HEADER_BITS)) | (1 << (32 - HEADER_BITS))] + pool[1:]
    near, left = pool[:3], skip
    for r in range(1, 8):
        left = left - lax.population_count(pool[r - 1])
        past = left > 0
        skip = jnp.where(past, left, skip)
        near = [jnp.where(past, a, b) for a, b in zip(pool[r:r + 3], near)] + near[8 - r:]
    x, bit = near[0], jnp.zeros(skip.shape, I32)
    for k in (16, 8, 4, 2, 1):
        left = skip - lax.population_count(_shr(x, 32 - k))
        past = left > 0
        skip, x = jnp.where(past, left, skip), jnp.where(past, _shl(x, k), x)
        bit = jnp.where(past, bit + k, bit)
    rest = [_skew(m, _sll(_shl(a, 1), bit) | _srl(b, 31 - bit), -1)
            for a, b in zip(near, near[1:])]
    if m.half:
        code[-1] = code[-1] | _shr(rest[0], 16)
        rest = [_shl(rest[0], 16) | _shr(rest[1], 16), _shl(rest[1], 16)]
    code += rest

    for t in range(m.tiles):
        zeros = []
        for run in (2 * t, 2 * t + 1):
            if run == 0:
                bits, end = code[0], 8
            else:
                allowed = _words_at(run, len(code) - 1)
                word, bit = _shr(end, 5), end & 31
                left, right = code[allowed[0]], code[allowed[0] + 1]
                for k in allowed[1:]:
                    here = word == k
                    left = jnp.where(here, code[k], left)
                    if k + 1 < len(code):
                        right = jnp.where(here, code[k + 1], right)
                bits, end = _sll(left, bit) | _srl(_shr(right, 1), 31 - bit), end + 8
            for _ in range(8):
                zeros.append(lax.clz(bits))
                bits, end = _sll(_shl(bits, 1), zeros[-1]), end + zeros[-1]
        signs = load(m.signs + t // 2)
        yield [(_shl(signs, 8 * (t % 2) + j) & SIGNS)
               | ((_shl(zeros[j], 24) | _shl(zeros[8 + j], 8)) ^ _i32(0x7F007F00)) for j in range(8)]


MESSAGES = {k: _messages(chunks) for k, chunks in CHUNKS.items()}
ENCODED = [(k, i) for k in CHUNKS for i in range(len(CHUNKS[k]))]
SENT = [(k, i) for k in "ABCDEF" for i in range(len(CHUNKS[STREAM[k]]))] + [("X", MOVED)]


def _steps():
    for step in SCHEDULE.split():
        step, _, chips = step.partition(":")
        name = step.rstrip("0123456789")
        digits = [int(d) for d in step[len(name):]]
        yield name, digits[0] if digits else None, digits[1:] or [0, 1], chips


def _body(x_hbm, out, own, terms, words, levels, ready, load_sems, send_sems, recv_sems, *buffers):
    outbox, inbox = dict(zip(CHUNKS, buffers)), dict(zip(STREAM, buffers[len(CHUNKS):]))
    me = lax.axis_index("i")
    neighbours = me ^ 1, 3 - me
    role = {"f": me == 0, "m": (me & 1) == 1, "l": me == 2}
    barrier = pltpu.get_barrier_semaphore()

    def signal(sem):
        for chip in neighbours:
            pl.semaphore_signal(sem, inc=1, device_id=(chip,), device_id_type=MESH)

    pl.when(me != 2)(lambda: signal(barrier))

    flip = (me == 3).astype(I32)
    half = flip, 1 - flip
    link = [jnp.where(h == 0, *neighbours) for h in half]
    place = [jnp.where(h == 0, (me ^ (me >> 1)) & 1, me >> 1) for h in half]

    def rows(k, u, row, n):
        a = 1 - place[u] if k in "abEF" else place[u]
        b = 1 - place[1 - u] if k in "acDF" else place[1 - u]
        return pl.ds(pl.multiple_of((4 * half[u] + 2 * a + b) * BLOCK + row, 16), n)

    loads = {}
    for k, i, halves, _ in _steps():
        k = k.rstrip("-")
        for u in halves if k in CHUNKS else ():
            if (k, i, u) not in loads:
                m = MESSAGES[k][i]
                loads[k, i, u] = pltpu.make_async_copy(
                    x_hbm.at[rows(k, u, m.row, m.rows)],
                    own.at[list(CHUNKS).index(k), u, pl.ds(m.row, m.rows)],
                    load_sems.at[len(loads)])
    waiting = list(loads.values())

    def copy(k, i, u, part, sending=False):
        m = MESSAGES[STREAM[k]][i]
        peer = link[u if k in "ABEF" else 1 - u]
        there = half[u] ^ (peer == 3).astype(I32) if sending else u
        cut, sent = 32 * APART.get((k, i), 0), 8 * m.pool + m.pool_rows
        lo, hi = {MAIN: (cut, sent), POOL_ROW: (sent, sent + 1), POOL_REST: (sent, 8 * m.pool + 8),
                  HIGH_BYTES: (8 * m.pool + 8, 8 * m.size), LOW: (0, cut)}[part]
        span, sem = m.at(0, lo, hi - lo), 3 * SENT.index((k, i)) + {MAIN: 0, LOW: 1}.get(part, 2)
        source = inbox["D"] if k == "F" else outbox[STREAM[k]]
        return pltpu.make_async_remote_copy(
            source.at[u, span], inbox[k].at[there, span], send_sems.at[u, sem],
            recv_sems.at[there, sem], device_id=(peer,), device_id_type=MESH)

    def on_demand(level, f):
        @pl.when(level > 0)
        def _():
            for part in (POOL_ROW, POOL_REST, HIGH_BYTES):
                pl.when(level == part)(functools.partial(f, part))

    arrived, unfinished = {}, []

    def arrive(k, i, u):
        if (k, i, u) not in arrived:
            m = MESSAGES[STREAM[k]][i]
            copy(k, i, u, MAIN).wait_recv()
            level = _shr(inbox[k][u, m.at(m.pool, 0, 1)][0, 0], 30)
            on_demand(level, lambda part: copy(k, i, u, part).wait_recv())
            arrived[k, i, u] = level
        return arrived[k, i, u]

    def pairs(m, t, lower):
        return pl.ds((m.row + TILE * t) // 2 + 8 * lower, 8)

    def receive(k, i):
        m, box = MESSAGES[STREAM[k]][i], inbox[k]
        verbatim = [arrive(k, i, u) == HIGH_BYTES for u in range(2)]

        def pool_row(r):
            return jnp.broadcast_to(box[:, m.at(m.pool, r, 1)], (2, 8, 128))

        @pl.when(jnp.logical_not(jnp.logical_and(*verbatim)))
        def _():
            pool = [pool_row(r) for r in range(8)]
            level = _shr(pool[0], 30)
            for r in range(m.pool_rows, 8):
                came = level == POOL_REST
                came = came | (level == POOL_ROW) if r == m.pool_rows else came
                pool[r] = jnp.where(came, pool[r], 0)
            for t, high in enumerate(_decode_high(m, lambda v: box[:, m.at(v)], pool)):
                for lower in range(2):
                    words[:, pairs(m, t, lower)] = jnp.concatenate(high[4 * lower:4 * lower + 4], axis=2)

        for u in range(2):
            @pl.when(verbatim[u])
            def _():
                for t in range(m.tiles):
                    high = jnp.concatenate([box[u, m.at(m.high(t, j))] for j in range(4)], axis=1)
                    words[u, pairs(m, t, 0)] = _shl(high & BYTES, 8)
                    words[u, pairs(m, t, 1)] = high & ~BYTES

        offset = _twice(_shr(pool_row(0), 32 - HEADER_BITS) & 0x7FF)
        for t in range(m.tiles):
            if t == m.tiles - APART.get((k, i), 0):
                for u in range(2):
                    copy(k, i, u, LOW).wait_recv()
            low = jnp.concatenate([box[:, m.at(m.low(t, j))] for j in range(4)], axis=2)
            for lower in range(2):
                x = ((_shr(low, 8 * lower) & BYTES) + (offset & BYTES)) & BYTES
                x = _swap(words[:, pairs(m, t, lower)] | x) - offset
                if k in "DEF":
                    for u in range(2):
                        row = m.row + TILE * t + 16 * lower
                        out[rows(k, u, row, 16)] = pltpu.bitcast(x[u], jnp.bfloat16)
                else:
                    terms["ABCX".index(k), :, pairs(m, t, lower)] = x

    def receive_term(k, i):
        if STREAM[k] != "a" or i != MOVED:
            return receive(k, i)
        comes = role["l"] if k == "X" else jnp.logical_not(role["f"])
        pl.when(comes)(lambda: receive(k, i))

        @pl.when(jnp.logical_not(comes))
        def _():
            m = MESSAGES["a"][i]
            terms["ABCX".index(k), :, pl.ds(m.row // 2, m.rows // 2)] = jnp.full(
                (2, m.rows // 2, N), SIGNS, I32)

    def encode_low(k, i, halves):
        m = MESSAGES[k][i]
        for u in halves:
            loads.pop((k, i, u)).wait()
        added = [(r, j) for r, j in SENT if r in TERMS[k]
                 and m.row <= MESSAGES[STREAM[r]][j].row < m.row + m.rows]
        for r, j in added:
            receive_term(r, j)
        for u in halves:
            for t in range(m.tiles):
                low = []
                for lower in range(2):
                    row = m.row + TILE * t + 16 * lower
                    x = own[list(CHUNKS).index(k), u, pl.ds(row, 16)]
                    for r in sorted({r for r, _ in added}):
                        term = terms["ABCX".index(r), u, pairs(m, t, lower)]
                        x = x + pltpu.bitcast(term, jnp.bfloat16).astype(jnp.float32)
                    rounded = x.astype(jnp.bfloat16)
                    if k == "t":
                        out[rows(k, u, row, 16)] = rounded
                    rounded = pltpu.bitcast(rounded, I32)
                    words[u, pairs(m, t, lower)] = rounded
                    low.append(_shl(rounded & BYTES, 8 * lower))
                    x = jnp.abs(x)
                    x = jnp.maximum(x[:, :256], x[:, 256:])
                    x = jnp.maximum(x[:, :128], x[:, 128:])
                    x = jnp.maximum(x[:8], x[8:])
                    top = x if row == m.row else jnp.maximum(top, x)
                low = _or(low)
                for j in range(4):
                    outbox[k][u, m.at(m.low(t, j))] = low[:, 128 * j:128 * (j + 1)]
            outbox[k][u, m.at(m.pool)] = pltpu.bitcast(top, I32)

    def encode(k, i):
        m, box = MESSAGES[k][i], outbox[k]
        if (k, i, 0) in loads:
            encode_low(k, i, [0, 1])
        top = _shr(box[:, m.at(m.pool)] + 0xFFFF, 16) & 0x7FFF
        for down in (1, 2, 4):
            other = pltpu.roll(top, down, 1)
            top = jnp.where(other > top, other, top)
        offset = _shr(0x7FFF - top, 4)
        wide = _twice(offset)

        def tile(t):
            x = [_swap(words[:, pairs(m, t, lower)] + wide) for lower in range(2)]
            return [x[j // 4][:, :, 128 * (j % 4):128 * (j % 4 + 1)] for j in range(8)]

        def store(v, x):
            box[:, m.at(v)] = x

        pool, needs = _encode_high(m, tile, store, _shl(offset, 32 - HEADER_BITS))
        store(m.pool, pool)
        for u, level in enumerate([jnp.max(needs[u]).astype(I32) for u in range(2)]):
            levels[u, ENCODED.index((k, i))] = level

            @pl.when(level > 0)
            def _():
                first = m.at(m.pool, 0, 1)
                box[u, first] = (box[u, first] & 0x3FFFFFFF) | _shl(level, 30)

                @pl.when(level == HIGH_BYTES)
                def _():
                    for t in range(m.tiles):
                        x = [_swap(words[u, pairs(m, t, lower)] + wide[u]) for lower in range(2)]
                        high = (_shr(x[0], 8) & BYTES) | (x[1] & ~BYTES)
                        for j in range(4):
                            box[u, m.at(m.high(t, j))] = high[:, 128 * j:128 * (j + 1)]

    def each_copy(k, i, u, f, low):
        level = arrive("D", i, u) if k == "F" else levels[u, ENCODED.index((STREAM[k], i))]

        def to(k):
            f(copy(k, i, u, MAIN, True))
            on_demand(level, lambda part: f(copy(k, i, u, part, True)))
            if low and (k, i) in APART:
                f(copy(k, i, u, LOW, True))

        if (k, i, u) == ("A", MOVED, 0):
            pl.when(role["m"])(lambda: to("X"))
            pl.when(jnp.logical_not(role["m"]))(lambda: to("A"))
        else:
            to(k)

    def finish_sends(keep):
        while len(unfinished) > keep:
            each_copy(*unfinished.pop(0), lambda c: c.wait_send(), True)

    def run(name, i, halves, chips):
        if name == "load":
            for c in waiting[:i]:
                c.start()
            del waiting[:i]
        elif name == "bar":
            pl.semaphore_wait(barrier, 1 if chips == "m" else 2)
        elif name == "go":
            signal(ready)
        elif name == "rdy":
            pl.semaphore_wait(ready, 1)
        elif name == "sent":
            finish_sends(2)
        elif name[0] in CHUNKS and name[1:] == "-":
            encode_low(name[0], i, halves)
        elif name[1:] == "-":
            for u in halves:
                copy(name[0], i, u, LOW, True).start()
        elif name in CHUNKS:
            encode(name, i)
        elif name in STREAM:
            for u in halves:
                each_copy(name, i, u, lambda c: c.start(), name == "F")
                if (name, i, u) not in unfinished:
                    unfinished.append((name, i, u))
        else:
            receive(name.upper(), i)

    for step in _steps():
        if step[-1]:
            chosen = functools.reduce(jnp.logical_or, [role[r] for r in step[-1]])
            pl.when(chosen)(functools.partial(run, *step))
        else:
            run(*step)
    finish_sends(0)
    assert not waiting and not loads


def pallas_dist_ar_i_i_m2048_n512_kernel(x: jax.Array):
    assert x.shape == (M, N) and x.dtype == jnp.float32

    def box(k):
        return pltpu.VMEM((2, 8 * sum(m.size for m in MESSAGES[k]), 128), I32)

    return pl.pallas_call(
        _body,
        out_shape=jax.ShapeDtypeStruct((M, N), jnp.bfloat16),
        in_specs=[pl.BlockSpec(memory_space=pltpu.HBM)],
        out_specs=pl.BlockSpec(memory_space=pltpu.VMEM),
        scratch_shapes=[
            pltpu.VMEM((4, 2, BLOCK, N), jnp.float32),
            pltpu.VMEM((4, 2, BLOCK // 2, N), I32),
            pltpu.VMEM((2, BLOCK // 2, N), I32),
            pltpu.SMEM((2, len(ENCODED)), I32),
            pltpu.SemaphoreType.REGULAR,
            pltpu.SemaphoreType.DMA((2 * len(ENCODED),)),
            pltpu.SemaphoreType.DMA((2, 3 * len(SENT))),
            pltpu.SemaphoreType.DMA((2, 3 * len(SENT))),
            *[box(k) for k in CHUNKS],
            *[box(k) for k in STREAM.values()],
        ],
        compiler_params=pltpu.CompilerParams(collective_id=0, disable_semaphore_checks=True),
    )(x)
```

```python
import functools
import operator

import jax
import jax.numpy as jnp
import numpy as np
from jax import lax
from jax.experimental import pallas as pl
from jax.experimental.pallas import tpu as pltpu

M, N = 2048, 512
BLOCK = M // 8
TILE = 32
I32 = jnp.int32
MESH = pl.DeviceIdType.MESH

CHUNKS = {"a": (1, 3, 3, 1), "b": (4, 3, 1), "c": (4, 3, 1), "t": (4, 4)}
STREAM = {"A": "a", "B": "b", "C": "c", "D": "t", "E": "t", "F": "t", "X": "a"}
TERMS = {"a": "", "b": "X", "c": "A", "t": "BC"}
APART = {("A", 0): 1, ("A", 1): 3, ("C", 0): 4, ("E", 0): 4, ("F", 1): 2}
MOVED = 3

SCHEDULE = """
    load4 bar:m bar:l go:l a-00 A-00:ml a-01 A-01:l load2 a0 A00:ml A01:l
    a-10 A-10:ml a-11 A-11:l rdy:m A-01:m A01:m A-11:m a1 bar:f A-0:f A0:f A-1:f A1
    load4 a2 A2 load a3 A3 b0 B0 c-0 C-0 c0 C0 b1 B1 b2 B2 c1 C1 c2 C2
    t-0 E-0 t0 D0 E0 t1 D1 E1 F0 d0 e0 F1 d1 e1 f0 sent f1
"""

HEADER_BITS = 13
ROOM = {1: (1, 4, (8,)), 3: (5, 2, (6, 6, 6, 6)), 4: (6, 5, (7, 7, 6, 6, 6))}
MAIN, POOL_ROW, POOL_REST, HIGH_BYTES, LOW = range(5)


def _i32(v):
    return np.array(v & 0xFFFFFFFF, np.uint32).view(np.int32)[()]


SIGNS, BYTES = _i32(0x80008000), _i32(0x00FF00FF)
_srl, _sll, _select = lax.shift_right_logical, lax.shift_left, lax.select


def _shr(x, k):
    return _srl(x, _i32(k)) if k else x


def _shl(x, k):
    return _sll(x, _i32(k)) if k else x


def _or(xs):
    return functools.reduce(operator.or_, xs)


def _row(like):
    return lax.broadcasted_iota(I32, like.shape, 1)


def _twice(offset):
    return jnp.concatenate([_shl(offset, 20) | _shl(offset, 4)] * 4, axis=2)


def _swap(x):
    return x ^ (_shr((x & _i32(0x7E807E80)) + _i32(0x01800180), 7) & _i32(0x01000100))


def _skew(m, x, sign):
    if m.tiles == 1:
        return x
    group, out = _row(x) & 3, x
    for g in range(1, 4):
        out = _select(group == g, pltpu.roll(x, 32 * g * sign % 128, 2), out)
    return out


def _sum_above(x):
    row, total = _row(x), x
    for k in (1, 2, 4):
        total = total + jnp.where(row >= k, pltpu.roll(total, k, 1), 0)
    return total - x


def _words_at(done, last):
    return range(done // 32, min((2 * done + 30) // 32, last) + 1)


class _Message:
    def __init__(self, row, tiles, start):
        self.row, self.tiles, self.rows, self.start = row, tiles, tiles * TILE, start
        units, self.pool_rows, self.runs = ROOM[tiles]
        self.full, self.half = divmod(units, 2)
        self.signs = 4 * tiles
        self.unary = self.signs + (tiles + 1) // 2
        self.pool = self.unary + self.full
        self.size = 8 * tiles + 1

    def low(self, t, j):
        return 4 * (self.tiles - 1 - t) + j

    def high(self, t, j):
        v = self.signs + 4 * t + j
        return v + (v >= self.pool)

    def at(self, v, row=0, rows=8):
        return pl.ds(8 * (self.start + v) + row, rows)


def _messages(chunks):
    out, row, start = [], 0, 0
    for tiles in chunks:
        out.append(_Message(row, tiles, start))
        row, start = row + out[-1].rows, start + out[-1].size
    assert row == BLOCK
    return out


def _encode_high(m, words, store, header):
    code = [[] for _ in range(m.full + m.half + 2)]
    spare, signs, done, zero = [], [], 0, jnp.zeros(header.shape, I32)
    for run in m.runs:
        upper, lower = [], []
        for j in range(run):
            w, index = next(words), done // 2 + j
            signs = [_or(signs + [_shr(w & SIGNS, index % 16)])]
            if index % 16 == 15:
                store(m.signs + index // 16, signs.pop())
            field = _shr(w, 8) & _i32(0x007F007F)
            fields = field if j == 0 else fields + field
            zeros = _i32(127 * (j + 1) * 0x10001) - fields
            upper.append(_srl(_i32(0x80000000 >> j), _shr(zeros, 16)))
            lower.append(_srl(_i32(0x80000000 >> j), zeros & 0xFFFF))
        for bits, length in ((_or(upper), _shr(zeros, 16) + run),
                             (_or(lower), (zeros & 0xFFFF) + run)):
            spare.append(32 - length)
            done += run
            if done == run:
                code[0].append(bits)
                end = length
                continue
            allowed = _words_at(done - run, len(code) - 1)
            word, bit = _shr(end, 5), end & 31
            left, right = _srl(bits, bit), _sll(_shl(bits, 1), 31 - bit)
            for k in allowed:
                here = word == k
                code[k].append(_select(here, left, zero))
                if k + 1 < len(code):
                    code[k + 1].append(_select(here, right, zero))
            spare.append(allowed[-1] - word)
            end = end + length
        code = [[_or(x)] if x else [] for x in code]
        spare = [_or(spare)]
    code = [x[0] if x else zero for x in code]
    for k in range(m.full):
        store(m.unary + k, code[k])
    rest = code[m.full:]
    if m.half:
        store(m.unary - 1, signs.pop() | (_shr(rest[0], 8) & 0xFF0000) | (_shr(rest[0], 16) & 0xFF))
        rest = [_shl(a, 16) | _shr(b, 16) for a, b in zip(rest, rest[1:])]

    length = end - (32 * m.full + 16 * m.half)
    length = _skew(m, jnp.where(length > 0, length, 0), 1)
    first, second = (_skew(m, x, 1) for x in rest)
    start = _sum_above(length) + HEADER_BITS
    word, bit, row = _shr(start, 5), start & 31, _row(start)
    pieces = (_srl(first, bit), _sll(_shl(first, 1), 31 - bit) | _srl(second, bit),
              _sll(_shl(second, 1), 31 - bit))
    pool = jnp.where(row == 0, header, 0)
    for down in range(8):
        which, x = ((row + down) & 7) - word, zero
        for k, piece in enumerate(pieces):
            x = _select(which == k, piece, x)
        pool = pool | (pltpu.roll(x, down, 1) if down else x)
    end = start + length
    fits = (spare[0] | (64 - length) | (256 - end)) >= 0
    level = jnp.where(end > 32 * m.pool_rows, float(POOL_ROW), float(MAIN))
    level = jnp.where(end > 32 * (m.pool_rows + 1), float(POOL_REST), level)
    return pool, jnp.where(fits, level, float(HIGH_BYTES))


def _decode_high(m, load, pool):
    code = [load(m.unary + k) for k in range(m.full)]
    if m.half:
        x = load(m.unary - 1)
        code.append(_shl(x & 0xFF0000, 8) | _shl(x & 0xFF, 16))
    ones = functools.reduce(operator.add, [lax.population_count(x) for x in code])
    skip = _sum_above(_skew(m, 16 * m.tiles - ones, 1)) + 1
    pool = [(pool[0] & _i32(0xFFFFFFFF >> HEADER_BITS)) | (1 << (32 - HEADER_BITS))] + pool[1:]
    near, left = pool[:3], skip
    for r in range(1, 8):
        left = left - lax.population_count(pool[r - 1])
        past = left > 0
        skip = _select(past, left, skip)
        near = [_select(past, a, b) for a, b in zip(pool[r:r + 3], near)] + near[8 - r:]
    x, bit = near[0], jnp.zeros(skip.shape, I32)
    for k in (16, 8, 4, 2, 1):
        left = skip - lax.population_count(_shr(x, 32 - k))
        past = left > 0
        skip, x = _select(past, left, skip), _select(past, _shl(x, k), x)
        bit = _select(past, bit + k, bit)
    rest = [_skew(m, _sll(_shl(a, 1), bit) | _srl(b, 31 - bit), -1)
            for a, b in zip(near, near[1:])]
    if m.half:
        code[-1] = code[-1] | _shr(rest[0], 16)
        rest = [_shl(rest[0], 16) | _shr(rest[1], 16), _shl(rest[1], 16)]
    code += rest

    done = 0
    for run in m.runs:
        zeros = []
        for _ in range(2):
            if done == 0:
                bits, end = code[0], run
            else:
                allowed = _words_at(done, len(code) - 1)
                word, bit = _shr(end, 5), end & 31
                left, right = code[allowed[0]], code[allowed[0] + 1]
                for k in allowed[1:]:
                    here = word == k
                    left = _select(here, code[k], left)
                    if k + 1 < len(code):
                        right = _select(here, code[k + 1], right)
                bits, end = _sll(left, bit) | _srl(_shr(right, 1), 31 - bit), end + run
            for _ in range(run):
                zeros.append(lax.clz(bits))
                bits, end = _sll(_shl(bits, 1), zeros[-1]), end + zeros[-1]
            done += run
        for j in range(run):
            index = done // 2 - run + j
            field = (_shl(zeros[j], 24) | _shl(zeros[run + j], 8)) ^ _i32(0x7F007F00)
            yield field | (_shl(load(m.signs + index // 16), index % 16) & SIGNS)


MESSAGES = {k: _messages(chunks) for k, chunks in CHUNKS.items()}
ENCODED = [(k, i) for k in CHUNKS for i in range(len(CHUNKS[k]))]
SENT = [(k, i) for k in "ABCDEF" for i in range(len(CHUNKS[STREAM[k]]))] + [("X", MOVED)]


def _steps():
    for step in SCHEDULE.split():
        step, _, chips = step.partition(":")
        name = step.rstrip("0123456789")
        digits = [int(d) for d in step[len(name):]]
        yield name, digits[0] if digits else None, digits[1:] or [0, 1], chips


def _body(x_hbm, out, own, terms, words, levels, ready, load_sems, send_sems, recv_sems, *buffers):
    outbox, inbox = dict(zip(CHUNKS, buffers)), dict(zip(STREAM, buffers[len(CHUNKS):]))
    me = lax.axis_index("i")
    neighbours = me ^ 1, 3 - me
    role = {"f": me == 0, "m": (me & 1) == 1, "l": me == 2}
    barrier = pltpu.get_barrier_semaphore()

    def signal(sem):
        for chip in neighbours:
            pl.semaphore_signal(sem, inc=1, device_id=(chip,), device_id_type=MESH)

    pl.when(me != 2)(lambda: signal(barrier))

    flip = (me == 3).astype(I32)
    half = flip, 1 - flip
    link = [jnp.where(h == 0, *neighbours) for h in half]
    place = [jnp.where(h == 0, (me ^ (me >> 1)) & 1, me >> 1) for h in half]
    owned = [4 * half[u] + 2 * place[u] + place[1 - u] for u in range(2)]
    block = [[(owned[u] ^ across) * BLOCK for across in range(4)] for u in range(2)]
    flipped = [(chip == 3).astype(I32) for chip in link]

    def rows(k, u, row, n):
        across = 2 * (k in "abEF") + (k in "acDF")
        return pl.ds(pl.multiple_of(block[u][across] + row, 16), n)

    loads = {}
    for k, i, halves, _ in _steps():
        k = k.rstrip("-")
        for u in halves if k in CHUNKS else ():
            if (k, i, u) not in loads:
                m = MESSAGES[k][i]
                loads[k, i, u] = pltpu.make_async_copy(
                    x_hbm.at[rows(k, u, m.row, m.rows)],
                    own.at[list(CHUNKS).index(k), u, pl.ds(m.row, m.rows)],
                    load_sems.at[len(loads)])
    waiting = list(loads.values())

    def copy(k, i, u, part, sending=False):
        m = MESSAGES[STREAM[k]][i]
        over = u if k in "ABEF" else 1 - u
        there = half[u] ^ flipped[over] if sending else u
        cut, sent = 32 * APART.get((k, i), 0), 8 * m.pool + m.pool_rows
        lo, hi = {MAIN: (cut, sent), POOL_ROW: (sent, sent + 1), POOL_REST: (sent, 8 * m.pool + 8),
                  HIGH_BYTES: (8 * m.pool + 8, 8 * m.size), LOW: (0, cut)}[part]
        span, sem = m.at(0, lo, hi - lo), 3 * SENT.index((k, i)) + {MAIN: 0, LOW: 1}.get(part, 2)
        source = inbox["D"] if k == "F" else outbox[STREAM[k]]
        return pltpu.make_async_remote_copy(
            source.at[u, span], inbox[k].at[there, span], send_sems.at[u, sem],
            recv_sems.at[there, sem], device_id=(link[over],), device_id_type=MESH)

    def on_demand(level, f):
        @pl.when(level > 0)
        def _():
            for part in (POOL_ROW, POOL_REST, HIGH_BYTES):
                pl.when(level == part)(functools.partial(f, part))

    arrived, unfinished = {}, []

    def arrive(k, i, u):
        if (k, i, u) not in arrived:
            m = MESSAGES[STREAM[k]][i]
            copy(k, i, u, MAIN).wait_recv()
            level = _shr(inbox[k][u, m.at(m.pool, 0, 1)][0, 0], 30)
            on_demand(level, lambda part: copy(k, i, u, part).wait_recv())
            arrived[k, i, u] = level
        return arrived[k, i, u]

    def pairs(m, t, lower):
        return pl.ds((m.row + TILE * t) // 2 + 8 * lower, 8)

    def receive(k, i):
        m, box = MESSAGES[STREAM[k]][i], inbox[k]
        verbatim = [arrive(k, i, u) == HIGH_BYTES for u in range(2)]

        def pool_row(r):
            return jnp.broadcast_to(box[:, m.at(m.pool, r, 1)], (2, 8, 128))

        @pl.when(jnp.logical_not(jnp.logical_and(*verbatim)))
        def _():
            pool = [pool_row(r) for r in range(8)]
            level = _shr(pool[0], 30)
            for r in range(m.pool_rows, 8):
                came = level == POOL_REST
                came = came | (level == POOL_ROW) if r == m.pool_rows else came
                pool[r] = jnp.where(came, pool[r], 0)
            for j, high in enumerate(_decode_high(m, lambda v: box[:, m.at(v)], pool)):
                words[:, pairs(m, j // 8, j // 4 % 2), pl.ds(128 * (j % 4), 128)] = high

        for u in range(2):
            @pl.when(verbatim[u])
            def _():
                for t in range(m.tiles):
                    high = jnp.concatenate([box[u, m.at(m.high(t, j))] for j in range(4)], axis=1)
                    words[u, pairs(m, t, 0)] = _shl(high & BYTES, 8)
                    words[u, pairs(m, t, 1)] = high & ~BYTES

        offset = _twice(_shr(pool_row(0), 32 - HEADER_BITS) & 0x7FF)
        for t in range(m.tiles):
            if t == m.tiles - APART.get((k, i), 0):
                for u in range(2):
                    copy(k, i, u, LOW).wait_recv()
            low = jnp.concatenate([box[:, m.at(m.low(t, j))] for j in range(4)], axis=2)
            for lower in range(2):
                x = ((_shr(low, 8 * lower) & BYTES) + (offset & BYTES)) & BYTES
                x = _swap(words[:, pairs(m, t, lower)] | x) - offset
                if k in "DEF":
                    for u in range(2):
                        row = m.row + TILE * t + 16 * lower
                        out[rows(k, u, row, 16)] = pltpu.bitcast(x[u], jnp.bfloat16)
                else:
                    terms["ABCX".index(k), :, pairs(m, t, lower)] = x

    def receive_term(k, i):
        if STREAM[k] != "a" or i != MOVED:
            return receive(k, i)
        comes = role["l"] if k == "X" else jnp.logical_not(role["f"])
        pl.when(comes)(lambda: receive(k, i))

        @pl.when(jnp.logical_not(comes))
        def _():
            m = MESSAGES["a"][i]
            terms["ABCX".index(k), :, pl.ds(m.row // 2, m.rows // 2)] = jnp.full(
                (2, m.rows // 2, N), SIGNS, I32)

    def encode_low(k, i, halves):
        m = MESSAGES[k][i]
        for u in halves:
            loads.pop((k, i, u)).wait()
        added = [(r, j) for r, j in SENT if r in TERMS[k]
                 and m.row <= MESSAGES[STREAM[r]][j].row < m.row + m.rows]
        for r, j in added:
            receive_term(r, j)
        for u in halves:
            for t in range(m.tiles):
                low = []
                for lower in range(2):
                    row = m.row + TILE * t + 16 * lower
                    x = own[list(CHUNKS).index(k), u, pl.ds(row, 16)]
                    for r in sorted({r for r, _ in added}):
                        term = terms["ABCX".index(r), u, pairs(m, t, lower)]
                        x = x + pltpu.bitcast(term, jnp.bfloat16).astype(jnp.float32)
                    rounded = x.astype(jnp.bfloat16)
                    if k == "t":
                        out[rows(k, u, row, 16)] = rounded
                    rounded = pltpu.bitcast(rounded, I32)
                    words[u, pairs(m, t, lower)] = rounded
                    low.append(_shl(rounded & BYTES, 8 * lower))
                    x = jnp.maximum(_shr(rounded, 16) & 0x7FFF, rounded & 0x7FFF)
                    x = jnp.maximum(x[:, :256], x[:, 256:])
                    x = jnp.maximum(x[:, :128], x[:, 128:])
                    top = x if row == m.row else jnp.maximum(top, x)
                low = _or(low)
                for j in range(4):
                    outbox[k][u, m.at(m.low(t, j))] = low[:, 128 * j:128 * (j + 1)]
            outbox[k][u, m.at(m.pool)] = top

    def encode(k, i):
        m, box = MESSAGES[k][i], outbox[k]
        if (k, i, 0) in loads:
            encode_low(k, i, [0, 1])
        top = box[:, m.at(m.pool)]
        for down in (1, 2, 4):
            top = jnp.maximum(top, pltpu.roll(top, down, 1))
        offset = _shr(0x7FFF - top, 4)
        wide = _twice(offset)

        def moved():
            for piece in range(2 * m.tiles):
                x = _swap(words[:, pairs(m, *divmod(piece, 2))] + wide)
                for j in range(4):
                    yield x[:, :, 128 * j:128 * (j + 1)]

        def store(v, x):
            box[:, m.at(v)] = x

        pool, needs = _encode_high(m, moved(), store, _shl(offset, 32 - HEADER_BITS))
        store(m.pool, pool)
        for u, level in enumerate([jnp.max(needs[u]).astype(I32) for u in range(2)]):
            levels[u, ENCODED.index((k, i))] = level

            @pl.when(level > 0)
            def _():
                first = m.at(m.pool, 0, 1)
                box[u, first] = (box[u, first] & 0x3FFFFFFF) | _shl(level, 30)

                @pl.when(level == HIGH_BYTES)
                def _():
                    for t in range(m.tiles):
                        x = [_swap(words[u, pairs(m, t, lower)] + wide[u]) for lower in range(2)]
                        high = (_shr(x[0], 8) & BYTES) | (x[1] & ~BYTES)
                        for j in range(4):
                            box[u, m.at(m.high(t, j))] = high[:, 128 * j:128 * (j + 1)]

    def each_copy(k, i, u, f, low):
        level = arrive("D", i, u) if k == "F" else levels[u, ENCODED.index((STREAM[k], i))]

        def to(k):
            f(copy(k, i, u, MAIN, True))
            on_demand(level, lambda part: f(copy(k, i, u, part, True)))
            if low and (k, i) in APART:
                f(copy(k, i, u, LOW, True))

        if (k, i, u) == ("A", MOVED, 0):
            pl.when(role["m"])(lambda: to("X"))
            pl.when(jnp.logical_not(role["m"]))(lambda: to("A"))
        else:
            to(k)

    def finish_sends(keep):
        while len(unfinished) > keep:
            each_copy(*unfinished.pop(0), lambda c: c.wait_send(), True)

    def run(name, i, halves, chips):
        if name == "load":
            for c in waiting[:i]:
                c.start()
            del waiting[:i]
        elif name == "bar":
            pl.semaphore_wait(barrier, 1 if chips == "m" else 2)
        elif name == "go":
            signal(ready)
        elif name == "rdy":
            pl.semaphore_wait(ready, 1)
        elif name == "sent":
            finish_sends(2)
        elif name[0] in CHUNKS and name[1:] == "-":
            encode_low(name[0], i, halves)
        elif name[1:] == "-":
            for u in halves:
                copy(name[0], i, u, LOW, True).start()
        elif name in CHUNKS:
            encode(name, i)
        elif name in STREAM:
            for u in halves:
                each_copy(name, i, u, lambda c: c.start(), name == "F")
                if (name, i, u) not in unfinished:
                    unfinished.append((name, i, u))
        else:
            receive(name.upper(), i)

    for step in _steps():
        if step[-1]:
            chosen = functools.reduce(jnp.logical_or, [role[r] for r in step[-1]])
            pl.when(chosen)(functools.partial(run, *step))
        else:
            run(*step)
    finish_sends(0)
    assert not waiting and not loads


def pallas_dist_ar_i_i_m2048_n512_kernel(x: jax.Array):
    assert x.shape == (M, N) and x.dtype == jnp.float32

    def box(k):
        return pltpu.VMEM((2, 8 * sum(m.size for m in MESSAGES[k]), 128), I32)

    return pl.pallas_call(
        _body,
        out_shape=jax.ShapeDtypeStruct((M, N), jnp.bfloat16),
        in_specs=[pl.BlockSpec(memory_space=pltpu.HBM)],
        out_specs=pl.BlockSpec(memory_space=pltpu.VMEM),
        scratch_shapes=[
            pltpu.VMEM((4, 2, BLOCK, N), jnp.float32),
            pltpu.VMEM((4, 2, BLOCK // 2, N), I32),
            pltpu.VMEM((2, BLOCK // 2, N), I32),
            pltpu.SMEM((2, len(ENCODED)), I32),
            pltpu.SemaphoreType.REGULAR,
            pltpu.SemaphoreType.DMA((2 * len(ENCODED),)),
            pltpu.SemaphoreType.DMA((2, 3 * len(SENT))),
            pltpu.SemaphoreType.DMA((2, 3 * len(SENT))),
            *[box(k) for k in CHUNKS],
            *[box(k) for k in STREAM.values()],
        ],
        compiler_params=pltpu.CompilerParams(collective_id=0, disable_semaphore_checks=True),
    )(x)
```
